```python
import numpy as np

kernel_name = "dist_sort_i_m128_n64"

def setup_inputs():
    return {"x": np.random.randn(512, 64).astype(np.float32)}

def reference(x: np.ndarray) -> np.ndarray:
    return np.sort(x, axis=0)
```

```python
import itertools
import jax
import jax.numpy as jnp
from jax import lax
from jax.experimental import pallas as pl
from jax.experimental.pallas import tpu as pltpu

MESH = pl.DeviceIdType.MESH
NT = (((1,), (1,)), ((), ()))

NET = {
    16: [(0, 13), (1, 12), (2, 15), (3, 14), (4, 8), (5, 6), (7, 11), (9, 10),
         (0, 5), (1, 7), (2, 9), (3, 4), (6, 13), (8, 14), (10, 15), (11, 12),
         (0, 1), (2, 3), (4, 5), (6, 8), (7, 9), (10, 11), (12, 13), (14, 15),
         (0, 2), (1, 3), (4, 10), (5, 11), (6, 7), (8, 9), (12, 14), (13, 15),
         (1, 2), (3, 12), (4, 6), (5, 7), (8, 10), (9, 11), (13, 14),
         (1, 4), (2, 6), (5, 8), (7, 10), (9, 13), (11, 14),
         (2, 4), (3, 6), (9, 12), (11, 13),
         (3, 5), (6, 8), (7, 9), (10, 12),
         (3, 4), (5, 6), (7, 8), (9, 10), (11, 12),
         (6, 7), (8, 9)],
    8: [(0, 2), (1, 3), (4, 6), (5, 7), (0, 4), (1, 5), (2, 6), (3, 7), (0, 1), (2, 3),
        (4, 5), (6, 7), (2, 4), (3, 5), (1, 4), (3, 6), (1, 2), (3, 4), (5, 6)],
    4: [(0, 2), (1, 3), (0, 1), (2, 3), (1, 2)],
    2: [(0, 1)],
}


def sub_iota(shape):
    return lax.broadcasted_iota(jnp.int32, shape, 0)


def perm(x, idx):
    return jnp.take_along_axis(x, idx, axis=0, mode="promise_in_bounds")


class Run:
    def __init__(self, regs, v, s, desc=False):
        self.r, self.v, self.s, self.desc = list(regs), list(v), list(s), desc

    def cmpx(self, a, b):
        lo, hi = jnp.minimum(a, b), jnp.maximum(a, b)
        return (hi, lo) if self.desc else (lo, hi)

    def exchange(self, k, victim=None):
        r = self.r
        if k in self.v:
            d = 1 << self.v.index(k)
            for i in range(len(r)):
                if not i & d:
                    r[i], r[i | d] = self.cmpx(r[i], r[i | d])
            return
        t, j = self.s.index(k), self.v.index(victim)
        si = sub_iota(r[0].shape)
        m, idx, d = (si & (1 << t)) == 0, si ^ (1 << t), 1 << j
        for i in range(len(r)):
            if not i & d:
                a, b = r[i], r[i | d]
                r[i], r[i | d] = self.cmpx(jnp.where(m, a, b), perm(jnp.where(m, b, a), idx))
        self.v[j], self.s[t] = k, victim

    def mirror(self, k):
        r = self.r
        t, j = self.s.index(k), self.v.index(0)
        vm = sum(1 << p for p, b in enumerate(self.v) if b < k)
        sm = sum(1 << p for p, b in enumerate(self.s) if b <= k)
        idx, d = sub_iota(r[0].shape) ^ sm, 1 << j
        new = list(r)
        for i in range(len(r)):
            if not i & d:
                new[i], new[i | d] = self.cmpx(r[i], perm(r[i ^ vm], idx))
        self.r = new
        self.v[j], self.s[t] = k, 0

    def swap(self, k, victim):
        r = self.r
        t, j = self.s.index(k), self.v.index(victim)
        si = sub_iota(r[0].shape)
        m, idx, d = (si & (1 << t)) == 0, si ^ (1 << t), 1 << j
        for i in range(len(r)):
            if not i & d:
                a, b = r[i], r[i | d]
                r[i], r[i | d] = jnp.where(m, a, perm(b, idx)), jnp.where(m, perm(a, idx), b)
        self.v[j], self.s[t] = k, victim

    def arrange(self, v, s):
        r = [None] * len(self.r)
        for i, x in enumerate(self.r):
            r[sum(((i >> j) & 1) << v.index(b) for j, b in enumerate(self.v))] = x
        if list(s) != self.s:
            si = sub_iota(r[0].shape)
            idx = sum(((si >> s.index(b)) & 1) << t for t, b in enumerate(self.s))
            r = [perm(x, idx) for x in r]
        self.r, self.v, self.s = r, list(v), list(s)
        return self


def sort_regs(regs, order, desc):
    n = len(regs).bit_length() - 1
    run = Run(regs, range(n), [n + o for o in order], desc)
    for a, b in NET[len(regs)]:
        run.r[a], run.r[b] = run.cmpx(run.r[a], run.r[b])
    for k in range(n, n + 3):
        run.mirror(k)
        for b in range(k - 1, -1, -1):
            run.exchange(b, b + 1)
    return run


def merge(d, lo, hi):
    r = d.r
    if lo is not None:
        r = [jnp.maximum(x, y) for x, y in zip(r, lo)]
    if hi is not None:
        r = [jnp.minimum(x, y) for x, y in zip(r, hi)]
    run = Run(r, d.v, d.s)
    first = True
    for b in range(len(d.v) + 2, -1, -1):
        if b in run.v:
            run.exchange(b)
        else:
            run.exchange(b, 0 if first else b + 1)
            first = False
    return run


def eye(m, k, dt):
    r = lax.broadcasted_iota(jnp.int32, (m, k), 0)
    c = lax.broadcasted_iota(jnp.int32, (m, k), 1)
    return jnp.where(r == c, 1.0, 0.0).astype(dt)


BIG = 2.0 ** 127


def to_key(x):
    k = jnp.minimum(jnp.maximum(x * 0.5, -BIG), BIG)
    return jnp.where(x != x, 1.5 * BIG, k)


def from_key(k):
    return jnp.where(k > BIG, jnp.nan, k * 2.0)


def split(t):
    return [t[8 * i:8 * i + 8] for i in range(t.shape[0] // 8)]


def mk(out_mode="mxu", dup=False, order=(0, 1, 2), flags=None):
    def f(x):
        xt = x.T

        def body(x_ref, o_ref, xbuf, sbuf, rbuf, mbuf, lsem, ssem, rsem, go):
            me = lax.axis_index("i")
            ld = pltpu.make_async_copy(x_ref, xbuf, lsem)
            ld.start()
            bs = pltpu.get_barrier_semaphore()
            sig = lambda s, d: pl.semaphore_signal(s, 1, device_id=(d,), device_id_type=MESH)
            rc = lambda k, dev: pltpu.make_async_remote_copy(
                sbuf, rbuf.at[k], ssem.at[k], rsem.at[k], device_id=(dev,), device_id_type=MESH)

            @pl.when(me != 2)
            def _():
                sig(bs, 2)

            @pl.when(me != 0)
            def _():
                sig(bs, 0)

            @pl.when(me == 0)
            def _():
                sig(bs, 1)
                sig(bs, 3)

            @pl.when(me == 2)
            def _():
                pl.semaphore_wait(bs, 3)
                sig(go, 1)
                sig(go, 3)

            inf = jnp.full((256, 128), jnp.inf, jnp.float32)
            mbuf[pl.ds(0, 256), :] = -inf
            mbuf[pl.ds(512, 256), :] = inf

            ld.wait()
            kb = pltpu.bitcast(to_key(xbuf[...]).astype(jnp.bfloat16), jnp.int32)
            sbuf[...] = kb

            @pl.when(me == 2)
            def _():
                rc(2, 0).start()
                rc(0, 1).start()
                pltpu.make_async_remote_copy(sbuf, rbuf.at[0], ssem.at[1], rsem.at[0], device_id=(3,), device_id_type=MESH).start()

            @pl.when((me & 1) == 1)
            def _():
                k = me >> 1
                pl.semaphore_wait(bs, 1)
                pltpu.make_async_remote_copy(sbuf, rbuf.at[k], ssem.at[0], rsem.at[k], device_id=(0,), device_id_type=MESH).start()
                pl.semaphore_wait(go, 1)
                rc(2, me ^ 2).start()
                pltpu.make_async_remote_copy(sbuf, rbuf.at[k], ssem.at[1], rsem.at[k], device_id=(2,), device_id_type=MESH).start()

            def sorted_run(words, desc):
                w = pltpu.bitcast(words, jnp.bfloat16)
                if dup:
                    w = jnp.concatenate([w, w], 0)
                t = lax.dot_general(eye(128, 128, jnp.bfloat16), w, NT, preferred_element_type=jnp.float32)
                return sort_regs(split(t), order, desc)

            nl = 128 if dup else 64
            own = sorted_run(kb, False)

            @pl.when(me == 0)
            def _():
                pl.semaphore_wait(bs, 3)
                pltpu.make_async_remote_copy(sbuf, rbuf.at[1], ssem.at[0], rsem.at[1], device_id=(1,), device_id_type=MESH).start()
                rc(1, 3).start()
                rc(2, 2).start()

            rc(0, 0).wait_recv()
            b = sorted_run(rbuf[0], True)
            for j, m in enumerate((merge(b, None, own.r), merge(b, own.r, None))):
                for i, r in enumerate(m.arrange(b.v, b.s).r):
                    mbuf[pl.ds(256 + 128 * j + 8 * i, 8), :nl] = r
            rc(1, 0).wait_recv()
            c = sorted_run(rbuf[1], True)
            base = pl.multiple_of(me * 128, 128)
            m = [[mbuf[pl.ds(base + 128 * j + 8 * i, 8), :nl] for i in range(16)] for j in range(3)]
            lo = merge(c, m[0], m[1]).arrange(c.v, c.s).r
            hi = merge(c, m[1], m[2]).arrange(c.v, c.s).r
            for k in range(3):
                rc(k, 0).wait_send()
            rc(2, 0).wait_recv()
            d = sorted_run(rbuf[2], True)
            res = merge(d, lo, hi)
            res.swap(3, 0)
            w = jnp.concatenate(res.arrange([3, 4, 5, 6], [0, 1, 2]).r, 0)
            if out_mode == "mxu":
                o = lax.dot_general(eye(64, nl, jnp.float32), w, NT, preferred_element_type=jnp.float32)
                o_ref[...] = from_key(o)
            else:
                o_ref[...] = from_key(w[:, :64].T)

        return pl.pallas_call(
            body, out_shape=jax.ShapeDtypeStruct(xt.shape, xt.dtype),
            in_specs=[pl.BlockSpec(memory_space=pl.ANY)], out_specs=pl.BlockSpec(memory_space=pltpu.VMEM),
            scratch_shapes=[pltpu.VMEM((64, 128), jnp.float32), pltpu.VMEM((32, 128), jnp.int32),
                            pltpu.VMEM((3, 32, 128), jnp.int32), pltpu.VMEM((768, 128), jnp.float32),
                            pltpu.SemaphoreType.DMA, pltpu.SemaphoreType.DMA((3,)), pltpu.SemaphoreType.DMA((3,)),
                            pltpu.SemaphoreType.REGULAR],
            compiler_params=pltpu.CompilerParams(collective_id=0, disable_semaphore_checks=True, flags=flags))(xt).T
    return f


def pallas_dist_sort_i_m128_n64_kernel(x):
    return mk(out_mode="xlu", order=(1, 0, 2))(x)
```

```python
import jax
import jax.numpy as jnp
from jax import lax
from jax.experimental import pallas as pl
from jax.experimental.pallas import tpu as pltpu

_FIRST, _LAST = 0, 2

_NETWORKS = {
    8: ((0, 2), (1, 3), (4, 6), (5, 7), (0, 4), (1, 5), (2, 6), (3, 7), (0, 1), (2, 3),
        (4, 5), (6, 7), (2, 4), (3, 5), (1, 4), (3, 6), (1, 2), (3, 4), (5, 6)),
    16: ((0, 13), (1, 12), (2, 15), (3, 14), (4, 8), (5, 6), (7, 11), (9, 10),
         (0, 5), (1, 7), (2, 9), (3, 4), (6, 13), (8, 14), (10, 15), (11, 12),
         (0, 1), (2, 3), (4, 5), (6, 8), (7, 9), (10, 11), (12, 13), (14, 15),
         (0, 2), (1, 3), (4, 10), (5, 11), (6, 7), (8, 9), (12, 14), (13, 15),
         (1, 2), (3, 12), (4, 6), (5, 7), (8, 10), (9, 11), (13, 14),
         (1, 4), (2, 6), (5, 8), (7, 10), (9, 13), (11, 14),
         (2, 4), (3, 6), (9, 12), (11, 13), (3, 5), (6, 8), (7, 9), (10, 12),
         (3, 4), (5, 6), (7, 8), (9, 10), (11, 12), (6, 7), (8, 9)),
}

_SUBLANE_GATHER = lax.GatherDimensionNumbers(
    offset_dims=(), collapsed_slice_dims=(0,), start_index_map=(0,),
    operand_batching_dims=(1,), start_indices_batching_dims=(1,))
_UPPER_HALF = -65536
_HUGE = 2.0**127


def _iota(axis, rows=8):
    return lax.broadcasted_iota(jnp.int32, (rows, 128), axis)


def _permute(reg, idx):
    return lax.gather(reg, idx.reshape(8, 128, 1), _SUBLANE_GATHER, (1, 1),
                      mode=lax.GatherScatterMode.PROMISE_IN_BOUNDS)


def _regs(x):
    return [x[i:i + 8] for i in range(0, x.shape[0], 8)]


def _stack(regs):
    return jnp.concatenate(regs, axis=0)


def _to_key(x):
    return jnp.where(x != x, 1.5 * _HUGE, jnp.minimum(jnp.maximum(x * 0.5, -_HUGE), _HUGE))


def _from_key(key):
    return jnp.where(key > _HUGE, jnp.nan, key * 2.0)


def _pack(x):
    return pltpu.bitcast(x.astype(jnp.bfloat16), jnp.int32)


def _pick_columns(onehot, w):
    step = onehot.shape[0] // 4
    out = []
    for i in range(0, 4 * step, step):
        out += _regs(lax.dot_general(onehot[i:i + step], w, (((1,), (1,)), ((), ())),
                                     preferred_element_type=jnp.float32))
    return out


def _transpose(w, rows):
    hit = _iota(0, rows) == (_iota(1, rows) & (rows - 1))
    return _pick_columns(jnp.where(hit, 1.0, 0.0).astype(w.dtype), w)


class _Run:
    def __init__(self, regs, reg_bits, sub_bits, descending=False):
        self.regs = list(regs)
        self.reg_bits = list(reg_bits)
        self.sub_bits = list(sub_bits)
        self.descending = descending

    def order(self, a, b):
        lo, hi = jnp.minimum(a, b), jnp.maximum(a, b)
        return (hi, lo) if self.descending else (lo, hi)

    def _update(self, bit, fn):
        d = 1 << self.reg_bits.index(bit)
        new = list(self.regs)
        for i in range(len(new)):
            if not i & d:
                new[i], new[i + d] = fn(i, d)
        self.regs = new

    def _trade(self, sub_bit, reg_bit):
        self.reg_bits[self.reg_bits.index(reg_bit)] = sub_bit
        self.sub_bits[self.sub_bits.index(sub_bit)] = reg_bit

    def swap(self, sub_bit, reg_bit):
        r, t = self.regs, 1 << self.sub_bits.index(sub_bit)
        clear, other = (_iota(0) & t) == 0, _iota(0) ^ t
        self._update(reg_bit, lambda i, d: (
            jnp.where(clear, r[i], _permute(r[i + d], other)),
            jnp.where(clear, _permute(r[i], other), r[i + d])))
        self._trade(sub_bit, reg_bit)
        return self

    def mirror(self, bit):
        r = self.regs
        flip_reg = sum(1 << j for j, b in enumerate(self.reg_bits) if b < bit)
        flip_sub = sum(1 << t for t, b in enumerate(self.sub_bits) if b <= bit)
        other = _iota(0) ^ flip_sub
        self._update(0, lambda i, d: self.order(r[i], _permute(r[i ^ flip_reg], other)))
        self._trade(bit, 0)

    def bitonic_merge(self, top, bottom=0):
        for bit in range(top, bottom - 1, -1):
            r = self.regs
            if bit in self.reg_bits:
                self._update(bit, lambda i, d: self.order(r[i], r[i + d]))
                continue
            t = 1 << self.sub_bits.index(bit)
            clear, other = (_iota(0) & t) == 0, _iota(0) ^ t
            self._update(bit + 1, lambda i, d: self.order(
                jnp.where(clear, r[i], r[i + d]),
                _permute(jnp.where(clear, r[i + d], r[i]), other)))
            self._trade(bit, bit + 1)
        return self

    def in_order(self):
        self.swap(3, 0)
        assert self.sub_bits == [0, 1, 2]
        return [self.regs[sum((i >> (b - 3) & 1) << j for j, b in enumerate(self.reg_bits))]
                for i in range(len(self.regs))]

    def folded(self):
        assert self.reg_bits == [0, 4, 5] and self.sub_bits == [1, 2, 3]
        first_copy = (_iota(1) & 16) == 0
        return [jnp.where(first_copy, *self.regs[i:i + 2]) for i in range(0, 8, 2)]


def _sort(regs, sublanes, descending):
    n = len(regs).bit_length() - 1
    run = _Run(regs, range(n), [n + t for t in sublanes], descending)
    for a, b in _NETWORKS[len(regs)]:
        run.regs[a], run.regs[b] = run.order(run.regs[a], run.regs[b])
    for bit in range(n, n + 3):
        run.mirror(bit)
        run.bitonic_merge(bit - 1)
    return run


def _clamp(new, lower, upper):
    if lower is not None:
        new = [jnp.maximum(a, b) for a, b in zip(new, lower)]
    if upper is not None:
        new = [jnp.minimum(a, b) for a, b in zip(new, upper)]
    return new


def _merge(new, lower, upper, sub_bits):
    top = len(new).bit_length() + 1
    return _Run(_clamp(new, lower, upper), range(3, top + 1), sub_bits).bitonic_merge(top)


def _merge_in_order(new, lower, upper):
    run = _merge(new, lower, upper, [0, 1, 2]).swap(3, 0)
    assert run.sub_bits == [1, 2, 0]
    idx = (_iota(0) >> 1) | ((_iota(0) & 1) << 2)
    return _stack([_permute(r, idx) for r in run.regs])


def _body(x_hbm, out_ref, x_ref, keys_tx, half_tx, run_tx, keys_rx, raw_rx, half_rx, run_rx,
          pair_ref, near_ref, pick_ref, idx_ref, load_sem, send_sems, recv_sems, go_sem):
    me = lax.axis_index("i")
    load = pltpu.make_async_copy(x_hbm, x_ref, load_sem)
    load.start()
    barrier = pltpu.get_barrier_semaphore()
    mesh = pl.DeviceIdType.MESH
    pieces = ((x_hbm.at[pl.ds(48, 16)], raw_rx), (half_tx, half_rx), (run_tx, run_rx))

    def signal(sem, chip):
        pl.semaphore_signal(sem, 1, device_id=(chip,), device_id_type=mesh)

    def to_neighbour(send_slot, recv_slot, chip):
        return pltpu.make_async_remote_copy(
            keys_tx, keys_rx.at[recv_slot], send_sems.at[send_slot], recv_sems.at[recv_slot],
            device_id=(chip,), device_id_type=mesh)

    def to_diagonal(piece, chip):
        return pltpu.make_async_remote_copy(
            *pieces[piece], send_sems.at[2 + piece], recv_sems.at[2 + piece],
            device_id=(chip,), device_id_type=mesh)

    def make_pieces(send_to=None):
        low = _iota(1) < 64
        keys = _regs(_to_key(x_ref[...]))
        half = [jnp.where(low, keys[i], keys[i + 1]) for i in (0, 2, 4, 4)]
        half_tx[...] = _pack(_stack(half))[:12]
        if send_to is not None:
            to_diagonal(1, send_to).start()
            keys[2] = _to_key(x_ref[pl.ds(16, 8), :])
        rest = [jnp.where(low, k, 0.0) if i in (1, 3, 5) else jnp.where(low, 0.0, k)
                for i, k in enumerate(keys)]
        w = _stack([rest[i + j] for i in range(0, 8, 2) for j in (0, 1, 0, 1)])
        run = _sort(_transpose(w, 64), (2, 1, 0), True).folded()
        run = [pltpu.bitcast(r, jnp.int32) for r in run]
        run_tx[...] = _stack([lax.shift_right_logical(run[i], 16) | (run[i + 1] & _UPPER_HALF)
                              for i in (0, 2)])
        if send_to is not None:
            to_diagonal(2, send_to).start()

    @pl.when(me == _LAST)
    def _():
        signal(barrier, _FIRST)
        pl.semaphore_wait(barrier, 3)
        to_diagonal(0, _FIRST).start()
        signal(go_sem, 1)
        signal(go_sem, 3)
        load.wait()
        make_pieces(_FIRST)
        keys_tx[...] = _pack(_to_key(x_ref[...]))
        to_neighbour(0, 0, 1).start()
        to_neighbour(1, 0, 3).start()

    @pl.when(me != _LAST)
    def _():
        signal(barrier, _LAST)

        @pl.when(me != _FIRST)
        def _():
            signal(barrier, _FIRST)

        @pl.when(me == _FIRST)
        def _():
            signal(barrier, 1)
            signal(barrier, 3)

        load.wait()
        keys_tx[...] = _pack(_to_key(x_ref[...]))

        @pl.when(me != _FIRST)
        def _():
            pl.semaphore_wait(barrier, 1)
            to_neighbour(0, me >> 1, _FIRST).start()

        make_pieces()

        @pl.when(me != _FIRST)
        def _():
            pl.semaphore_wait(go_sem, 1)
            for piece in range(3):
                to_diagonal(piece, me ^ 2).start()
            to_neighbour(1, me >> 1, _LAST).start()

    def sorted_shard(words, descending):
        w = _stack([pltpu.bitcast(r, jnp.bfloat16) for r in _regs(words) for _ in range(2)])
        return _sort(_transpose(w, 128), (0, 2, 1), descending).in_order()

    near_ref[pl.ds(0, 128), :] = _stack(sorted_shard(keys_tx[...], False))
    pair_ref[pl.ds(0, 256), :] = jnp.full((256, 128), -jnp.inf, jnp.float32)
    pair_ref[pl.ds(512, 256), :] = jnp.full((256, 128), jnp.inf, jnp.float32)
    row = _iota(0, 96) + 32
    lane = (row & 103) | ((row & 8) << 1) | ((row & 16) >> 1)
    pick_ref[...] = jnp.where(_iota(1, 96) == lane, 1.0, 0.0)
    idx_ref[...] = _iota(0, 32) >> 2

    @pl.when(me == _FIRST)
    def _():
        pl.semaphore_wait(barrier, 3)
        to_neighbour(0, 1, 1).start()
        to_neighbour(1, 1, 3).start()
        for piece in range(3):
            to_diagonal(piece, _LAST).start()

    to_neighbour(0, 0, me).wait_recv()
    new, own = sorted_shard(keys_rx[0], True), _regs(near_ref[pl.ds(0, 128), :])
    pair_ref[pl.ds(256, 128), :] = _merge_in_order(new, None, own)
    pair_ref[pl.ds(384, 128), :] = _merge_in_order(new, own, None)
    to_neighbour(1, 1, me).wait_recv()
    new = sorted_shard(keys_rx[1], True)
    pair = [_regs(pair_ref[pl.ds(pl.multiple_of((me + j) * 128, 128), 128), :]) for j in range(3)]
    near_ref[pl.ds(0, 128), :] = _merge_in_order(new, pair[0], pair[1])
    near_ref[pl.ds(128, 128), :] = _merge_in_order(new, pair[1], pair[2])
    to_neighbour(0, 0, me).wait_send()
    to_neighbour(1, 1, me).wait_send()

    to_diagonal(0, me).wait()
    raw = jnp.where(_iota(1, 16) < 64, _to_key(raw_rx[...]), 0.0).astype(jnp.bfloat16)

    def finish(lowest_quarter, diagonal):
        to_diagonal(1, diagonal).wait_recv()
        sent_here = ((_iota(0) >> 2) ^ (_iota(1) >> 6)) == 0
        w = []
        for start, offset in ((0, 0), (0, 4), (4, 4)):
            words = _permute(half_rx[pl.ds(start, 8), :], (_iota(0) & 3) + offset)
            w += [pltpu.bitcast(jnp.where(sent_here, words, 0), jnp.bfloat16)] * 2
        half = _transpose(_stack(w + [raw, raw]), 64)
        to_diagonal(1, diagonal).wait_send()
        half = _sort(half, (0, 2, 1), True).in_order()
        near = [None if lowest_quarter and j < 2 else _regs(near_ref[pl.ds(64 * j, 64), :])
                for j in range(4)]
        merged = [None if hi is None else _merge(half, lo, hi, [0, 1, 2]).folded()
                  for lo, hi in zip(near, near[1:])]

        to_diagonal(2, diagonal).wait()
        run = []
        for words in _regs(run_rx[...]):
            run += [pltpu.bitcast(words << 16, jnp.float32),
                    pltpu.bitcast(words & _UPPER_HALF, jnp.float32)]
        rows = []
        for lo, hi in zip(merged, merged[1:]):
            block = _Run(_clamp(run, lo, hi), [4, 5], [1, 2, 3]).bitonic_merge(5, 1)
            assert block.reg_bits == [1, 5] and block.sub_bits == [2, 3, 4]
            for i in (0, 2):
                rows += [jnp.where((_iota(0) & 2) == 0, _permute(block.regs[i], idx),
                                   _permute(block.regs[i + 1], idx))
                         for idx in _regs(idx_ref[...])]
        w = _stack(rows)
        head = _regs(w[:, :32].T)
        cols = [head[i] for i in (0, 2, 1, 3)] + _pick_columns(pick_ref[...], w)
        even = (_iota(1) & 1) == 0
        out_ref[...] = _from_key(_stack([
            jnp.where(even, jnp.minimum(a, b), jnp.maximum(a, b))
            for a, b in zip(cols[::2], cols[1::2])]))

    pl.when(me != 0)(lambda: finish(False, me ^ 2))
    pl.when(me == 0)(lambda: finish(True, 2))


def pallas_dist_sort_i_m128_n64_kernel(x: jax.Array):
    def vmem(rows, dtype):
        return pltpu.VMEM((rows, 128), dtype)

    out = pl.pallas_call(
        _body,
        out_shape=jax.ShapeDtypeStruct((64, 128), jnp.float32),
        in_specs=[pl.BlockSpec(memory_space=pl.ANY)],
        out_specs=pl.BlockSpec(memory_space=pltpu.VMEM),
        scratch_shapes=[
            vmem(64, jnp.float32),
            vmem(32, jnp.int32),
            vmem(12, jnp.int32),
            vmem(16, jnp.int32),
            pltpu.VMEM((2, 32, 128), jnp.int32),
            vmem(16, jnp.float32),
            vmem(12, jnp.int32),
            vmem(16, jnp.int32),
            vmem(768, jnp.float32),
            vmem(256, jnp.float32),
            vmem(96, jnp.float32),
            vmem(32, jnp.int32),
            pltpu.SemaphoreType.DMA,
            pltpu.SemaphoreType.DMA((5,)),
            pltpu.SemaphoreType.DMA((5,)),
            pltpu.SemaphoreType.REGULAR,
        ],
        compiler_params=pltpu.CompilerParams(collective_id=0, disable_semaphore_checks=True),
    )(x.T)
    return out.T
```

```python
import jax
import jax.numpy as jnp
from jax import lax
from jax.experimental import pallas as pl
from jax.experimental.pallas import tpu as pltpu

_FIRST, _LAST = 0, 2

_NETWORKS = {
    8: ((0, 2), (1, 3), (4, 6), (5, 7), (0, 4), (1, 5), (2, 6), (3, 7), (0, 1), (2, 3),
        (4, 5), (6, 7), (2, 4), (3, 5), (1, 4), (3, 6), (1, 2), (3, 4), (5, 6)),
    16: ((0, 13), (1, 12), (2, 15), (3, 14), (4, 8), (5, 6), (7, 11), (9, 10),
         (0, 5), (1, 7), (2, 9), (3, 4), (6, 13), (8, 14), (10, 15), (11, 12),
         (0, 1), (2, 3), (4, 5), (6, 8), (7, 9), (10, 11), (12, 13), (14, 15),
         (0, 2), (1, 3), (4, 10), (5, 11), (6, 7), (8, 9), (12, 14), (13, 15),
         (1, 2), (3, 12), (4, 6), (5, 7), (8, 10), (9, 11), (13, 14),
         (1, 4), (2, 6), (5, 8), (7, 10), (9, 13), (11, 14),
         (2, 4), (3, 6), (9, 12), (11, 13), (3, 5), (6, 8), (7, 9), (10, 12),
         (3, 4), (5, 6), (7, 8), (9, 10), (11, 12), (6, 7), (8, 9)),
}

_SUBLANE_GATHER = lax.GatherDimensionNumbers(
    offset_dims=(), collapsed_slice_dims=(0,), start_index_map=(0,),
    operand_batching_dims=(1,), start_indices_batching_dims=(1,))
_UPPER_HALF = -65536
_INF_KEY = 2.0**127
_MAX_KEY = _INF_KEY * (1 - 2.0**-8)


def _iota(axis, rows=8):
    return lax.broadcasted_iota(jnp.int32, (rows, 128), axis)


def _permute(reg, idx):
    return lax.gather(reg, idx.reshape(8, 128, 1), _SUBLANE_GATHER, (1, 1),
                      mode=lax.GatherScatterMode.PROMISE_IN_BOUNDS)


def _regs(x):
    return [x[i:i + 8] for i in range(0, x.shape[0], 8)]


def _stack(regs):
    return jnp.concatenate(regs, axis=0)


def _to_key(x):
    def clip(v, bound):
        return jnp.minimum(jnp.maximum(v, -bound), bound)

    return jnp.where(jnp.isfinite(x), clip(x * 0.5, _MAX_KEY),
                     jnp.where(x != x, 1.5 * _INF_KEY, clip(x, _INF_KEY)))


def _from_key(key):
    return jnp.where(key > _INF_KEY, jnp.nan, key * 2.0)


def _pack(x):
    return pltpu.bitcast(x.astype(jnp.bfloat16), jnp.int32)


def _pick_columns(onehot, w):
    step = onehot.shape[0] // 4
    out = []
    for i in range(0, 4 * step, step):
        out += _regs(lax.dot_general(onehot[i:i + step], w, (((1,), (1,)), ((), ())),
                                     preferred_element_type=jnp.float32))
    return out


def _transpose(w, rows):
    hit = _iota(0, rows) == (_iota(1, rows) & (rows - 1))
    return _pick_columns(jnp.where(hit, 1.0, 0.0).astype(w.dtype), w)


class _Run:
    def __init__(self, regs, reg_bits, sub_bits, descending=False):
        self.regs = list(regs)
        self.reg_bits = list(reg_bits)
        self.sub_bits = list(sub_bits)
        self.descending = descending

    def order(self, a, b):
        lo, hi = jnp.minimum(a, b), jnp.maximum(a, b)
        return (hi, lo) if self.descending else (lo, hi)

    def _update(self, bit, fn):
        d = 1 << self.reg_bits.index(bit)
        new = list(self.regs)
        for i in range(len(new)):
            if not i & d:
                new[i], new[i + d] = fn(i, d)
        self.regs = new

    def _trade(self, sub_bit, reg_bit):
        self.reg_bits[self.reg_bits.index(reg_bit)] = sub_bit
        self.sub_bits[self.sub_bits.index(sub_bit)] = reg_bit

    def swap(self, sub_bit, reg_bit):
        r, t = self.regs, 1 << self.sub_bits.index(sub_bit)
        clear, other = (_iota(0) & t) == 0, _iota(0) ^ t
        self._update(reg_bit, lambda i, d: (
            jnp.where(clear, r[i], _permute(r[i + d], other)),
            jnp.where(clear, _permute(r[i], other), r[i + d])))
        self._trade(sub_bit, reg_bit)
        return self

    def mirror(self, bit):
        r = self.regs
        flip_reg = sum(1 << j for j, b in enumerate(self.reg_bits) if b < bit)
        flip_sub = sum(1 << t for t, b in enumerate(self.sub_bits) if b <= bit)
        other = _iota(0) ^ flip_sub
        self._update(0, lambda i, d: self.order(r[i], _permute(r[i ^ flip_reg], other)))
        self._trade(bit, 0)

    def bitonic_merge(self, top, bottom=0):
        for bit in range(top, bottom - 1, -1):
            r = self.regs
            if bit in self.reg_bits:
                self._update(bit, lambda i, d: self.order(r[i], r[i + d]))
                continue
            t = 1 << self.sub_bits.index(bit)
            clear, other = (_iota(0) & t) == 0, _iota(0) ^ t
            self._update(bit + 1, lambda i, d: self.order(
                jnp.where(clear, r[i], r[i + d]),
                _permute(jnp.where(clear, r[i + d], r[i]), other)))
            self._trade(bit, bit + 1)
        return self

    def in_order(self):
        self.swap(3, 0)
        assert self.sub_bits == [0, 1, 2]
        return [self.regs[sum((i >> (b - 3) & 1) << j for j, b in enumerate(self.reg_bits))]
                for i in range(len(self.regs))]

    def folded(self):
        assert self.reg_bits == [0, 4, 5] and self.sub_bits == [1, 2, 3]
        first_copy = (_iota(1) & 16) == 0
        return [jnp.where(first_copy, *self.regs[i:i + 2]) for i in range(0, 8, 2)]


def _sort(regs, sublanes, descending):
    n = len(regs).bit_length() - 1
    run = _Run(regs, range(n), [n + t for t in sublanes], descending)
    for a, b in _NETWORKS[len(regs)]:
        run.regs[a], run.regs[b] = run.order(run.regs[a], run.regs[b])
    for bit in range(n, n + 3):
        run.mirror(bit)
        run.bitonic_merge(bit - 1)
    return run


def _clamp(new, lower, upper):
    if lower is not None:
        new = [jnp.maximum(a, b) for a, b in zip(new, lower)]
    if upper is not None:
        new = [jnp.minimum(a, b) for a, b in zip(new, upper)]
    return new


def _merge(new, lower, upper, sub_bits):
    top = len(new).bit_length() + 1
    return _Run(_clamp(new, lower, upper), range(3, top + 1), sub_bits).bitonic_merge(top)


def _merge_in_order(new, lower, upper):
    run = _merge(new, lower, upper, [0, 1, 2]).swap(3, 0)
    assert run.sub_bits == [1, 2, 0]
    idx = (_iota(0) >> 1) | ((_iota(0) & 1) << 2)
    return _stack([_permute(r, idx) for r in run.regs])


def _body(x_hbm, out_ref, x_ref, keys_tx, half_tx, run_tx, keys_rx, raw_rx, half_rx, run_rx,
          pair_ref, near_ref, pick_ref, idx_ref, load_sem, send_sems, recv_sems, go_sem):
    me = lax.axis_index("i")
    load = pltpu.make_async_copy(x_hbm, x_ref, load_sem)
    load.start()
    barrier = pltpu.get_barrier_semaphore()
    mesh = pl.DeviceIdType.MESH
    pieces = ((x_hbm.at[pl.ds(48, 16)], raw_rx), (half_tx, half_rx), (run_tx, run_rx))

    def signal(sem, chip):
        pl.semaphore_signal(sem, 1, device_id=(chip,), device_id_type=mesh)

    def to_neighbour(send_slot, recv_slot, chip=0):
        return pltpu.make_async_remote_copy(
            keys_tx, keys_rx.at[recv_slot], send_sems.at[send_slot], recv_sems.at[recv_slot],
            device_id=(chip,), device_id_type=mesh)

    def to_diagonal(piece, chip=0):
        return pltpu.make_async_remote_copy(
            *pieces[piece], send_sems.at[2 + piece], recv_sems.at[2 + piece],
            device_id=(chip,), device_id_type=mesh)

    def make_pieces(send_to=None):
        low = _iota(1) < 64

        def group(g):
            return _regs(x_ref[pl.ds(16 * g, 16), :])

        def other_half(g):
            if g == 3:
                return [jnp.where(low, 0.0, _to_key(r)) for r in group(g)] * 2
            key = _to_key(jnp.where(low, *group(g)[::-1]))
            return [jnp.where(low, 0.0, key), jnp.where(low, key, 0.0)] * 2

        half = [_to_key(jnp.where(low, *group(g))) for g in range(3)]
        half_tx[...] = _pack(_stack(half + half[2:]))[:12]
        upper = other_half(2) + other_half(3)
        if send_to is not None:
            to_diagonal(1, send_to).start()
        w = _stack(other_half(0) + other_half(1) + upper)
        run = _sort(_transpose(w, 64), (2, 1, 0), True).folded()
        run = [pltpu.bitcast(r, jnp.int32) for r in run]
        run_tx[...] = _stack([lax.shift_right_logical(run[i], 16) | (run[i + 1] & _UPPER_HALF)
                              for i in (0, 2)])
        if send_to is not None:
            to_diagonal(2, send_to).start()

    @pl.when(me == _LAST)
    def _():
        signal(barrier, _FIRST)
        pl.semaphore_wait(barrier, 3)
        to_diagonal(0, _FIRST).start()
        signal(go_sem, 1)
        signal(go_sem, 3)
        load.wait()
        make_pieces(_FIRST)
        keys_tx[...] = _pack(_to_key(x_ref[...]))
        to_neighbour(0, 0, 1).start()
        to_neighbour(1, 0, 3).start()

    @pl.when(me != _LAST)
    def _():
        signal(barrier, _LAST)

        @pl.when(me != _FIRST)
        def _():
            signal(barrier, _FIRST)

        @pl.when(me == _FIRST)
        def _():
            signal(barrier, 1)
            signal(barrier, 3)

        load.wait()
        keys_tx[...] = _pack(_to_key(x_ref[...]))

        @pl.when(me != _FIRST)
        def _():
            pl.semaphore_wait(barrier, 1)
            to_neighbour(0, me >> 1, _FIRST).start()

        make_pieces()

        for chip in (1, 3):
            @pl.when(me == chip)
            def _():
                pl.semaphore_wait(go_sem, 1)
                for piece in range(3):
                    to_diagonal(piece, chip ^ 2).start()
                to_neighbour(1, chip >> 1, _LAST).start()

    def sorted_shard(words, descending):
        w = _stack([pltpu.bitcast(r, jnp.bfloat16) for r in _regs(words) for _ in range(2)])
        return _sort(_transpose(w, 128), (0, 2, 1), descending).in_order()

    near_ref[pl.ds(0, 128), :] = _stack(sorted_shard(keys_tx[...], False))
    pair_ref[pl.ds(0, 256), :] = jnp.full((256, 128), -jnp.inf, jnp.float32)
    pair_ref[pl.ds(512, 256), :] = jnp.full((256, 128), jnp.inf, jnp.float32)
    row = _iota(0, 96) + 32
    lane = (row & 103) | ((row & 8) << 1) | ((row & 16) >> 1)
    pick_ref[...] = jnp.where(_iota(1, 96) == lane, 1.0, 0.0)
    idx_ref[...] = _iota(0, 32) >> 2

    @pl.when(me == _FIRST)
    def _():
        pl.semaphore_wait(barrier, 3)
        to_neighbour(0, 1, 1).start()
        to_neighbour(1, 1, 3).start()
        for piece in range(3):
            to_diagonal(piece, _LAST).start()

    to_neighbour(0, 0).wait_recv()
    new, own = sorted_shard(keys_rx[0], True), _regs(near_ref[pl.ds(0, 128), :])
    pair_ref[pl.ds(256, 128), :] = _merge_in_order(new, None, own)
    pair_ref[pl.ds(384, 128), :] = _merge_in_order(new, own, None)
    to_neighbour(1, 1).wait_recv()
    new = sorted_shard(keys_rx[1], True)
    pair = [_regs(pair_ref[pl.ds(pl.multiple_of((me + j) * 128, 128), 128), :]) for j in range(3)]
    near_ref[pl.ds(0, 128), :] = _merge_in_order(new, pair[0], pair[1])
    near_ref[pl.ds(128, 128), :] = _merge_in_order(new, pair[1], pair[2])
    to_neighbour(0, 0).wait_send()
    to_neighbour(1, 1).wait_send()

    to_diagonal(0).wait()
    raw = jnp.where(_iota(1, 16) < 64, _to_key(raw_rx[...]), 0.0).astype(jnp.bfloat16)

    def finish(lowest_quarter):
        to_diagonal(1).wait_recv()
        sent_here = ((_iota(0) >> 2) ^ (_iota(1) >> 6)) == 0
        w = []
        for start, offset in ((0, 0), (0, 4), (4, 4)):
            words = _permute(half_rx[pl.ds(start, 8), :], (_iota(0) & 3) + offset)
            w += [pltpu.bitcast(jnp.where(sent_here, words, 0), jnp.bfloat16)] * 2
        half = _transpose(_stack(w + [raw, raw]), 64)
        to_diagonal(1).wait_send()
        half = _sort(half, (0, 2, 1), True).in_order()
        near = [None if lowest_quarter and j < 2 else _regs(near_ref[pl.ds(64 * j, 64), :])
                for j in range(4)]
        merged = [None if hi is None else _merge(half, lo, hi, [0, 1, 2]).folded()
                  for lo, hi in zip(near, near[1:])]

        to_diagonal(2).wait()
        run = []
        for words in _regs(run_rx[...]):
            run += [pltpu.bitcast(words << 16, jnp.float32),
                    pltpu.bitcast(words & _UPPER_HALF, jnp.float32)]
        rows = []
        for lo, hi in zip(merged, merged[1:]):
            block = _Run(_clamp(run, lo, hi), [4, 5], [1, 2, 3]).bitonic_merge(5, 1)
            assert block.reg_bits == [1, 5] and block.sub_bits == [2, 3, 4]
            for i in (0, 2):
                rows += [jnp.where((_iota(0) & 2) == 0, _permute(block.regs[i], idx),
                                   _permute(block.regs[i + 1], idx))
                         for idx in _regs(idx_ref[...])]
        w = _stack(rows)
        head = _regs(w[:, :32].T)
        cols = [head[i] for i in (0, 2, 1, 3)] + _pick_columns(pick_ref[...], w)
        even = (_iota(1) & 1) == 0
        out_ref[...] = _from_key(_stack([
            jnp.where(even, jnp.minimum(a, b), jnp.maximum(a, b))
            for a, b in zip(cols[::2], cols[1::2])]))

    pl.when(me != 0)(lambda: finish(False))
    pl.when(me == 0)(lambda: finish(True))


def pallas_dist_sort_i_m128_n64_kernel(x: jax.Array):
    def vmem(rows, dtype):
        return pltpu.VMEM((rows, 128), dtype)

    out = pl.pallas_call(
        _body,
        out_shape=jax.ShapeDtypeStruct((64, 128), jnp.float32),
        in_specs=[pl.BlockSpec(memory_space=pl.ANY)],
        out_specs=pl.BlockSpec(memory_space=pltpu.VMEM),
        scratch_shapes=[
            vmem(64, jnp.float32),
            vmem(32, jnp.int32),
            vmem(12, jnp.int32),
            vmem(16, jnp.int32),
            pltpu.VMEM((2, 32, 128), jnp.int32),
            vmem(16, jnp.float32),
            vmem(12, jnp.int32),
            vmem(16, jnp.int32),
            vmem(768, jnp.float32),
            vmem(256, jnp.float32),
            vmem(96, jnp.float32),
            vmem(32, jnp.int32),
            pltpu.SemaphoreType.DMA,
            pltpu.SemaphoreType.DMA((5,)),
            pltpu.SemaphoreType.DMA((5,)),
            pltpu.SemaphoreType.REGULAR,
        ],
        compiler_params=pltpu.CompilerParams(collective_id=0, disable_semaphore_checks=True),
    )(x.T)
    return out.T
```
